```python
import numpy as np

kernel_name = "dist_ar_xy_y_m1024_n512"

def setup_inputs():
    return {"x": np.random.randn(2048, 512).astype(np.float32)}

def reference(x: np.ndarray) -> np.ndarray:
    return x.reshape(2, 1024, 512).sum(axis=0)
```

```python
import jax
import jax.numpy as jnp
from jax import lax
from jax.experimental import pallas as pl
from jax.experimental.pallas import tpu as pltpu

M, N = 1024, 512
ROWS = 16
NF, NP = 29, 6
LAG = 6
MESH = pl.DeviceIdType.MESH


def _body(x_hbm, o_ref, x_own, x_other, send, recv_y, recv_x,
          load_sems, ysend_sem, yrecv_sems, xsend_sem, xrecv_sems, ready_sem):
    mx, my = lax.axis_index("x"), lax.axis_index("y")
    ypeer, xpeer = (mx, 1 - my), (1 - mx, my)
    is_b = (mx == 0) & (my == 1)
    is_d = (mx == 1) & (my == 1)

    barrier = pltpu.get_barrier_semaphore()
    pl.semaphore_signal(barrier, 1, device_id=ypeer, device_id_type=MESH)

    @pl.when(jnp.logical_not(is_d))
    def _():
        pl.semaphore_signal(barrier, 1, device_id=xpeer, device_id_type=MESH)

    own0 = mx * ((NF + NP) * ROWS)
    other0 = (1 - mx) * ((NF + NP) * ROWS)

    def row0(i):
        r = own0 + i * ROWS if i < NF else i * ROWS
        return pl.multiple_of(r, ROWS) if i < NF else r

    def chunk(ref, i):
        return ref.at[pl.ds(i * ROWS, ROWS)]

    loads = [pltpu.make_async_copy(x_hbm.at[pl.ds(row0(i), ROWS)], chunk(x_own, i), load_sems.at[i])
             for i in range(NF + NP)]
    load_other = pltpu.make_async_copy(
        x_hbm.at[pl.ds(pl.multiple_of(other0, ROWS), NF * ROWS)], x_other, load_sems.at[NF + NP])
    for c in loads:
        c.start()
    load_other.start()

    ys = [pltpu.make_async_remote_copy(chunk(send, i), chunk(recv_y, i), ysend_sem, yrecv_sems.at[i],
                                       device_id=ypeer, device_id_type=MESH) for i in range(NF + NP)]
    xs = [pltpu.make_async_remote_copy(chunk(recv_y, i), chunk(recv_x, i), xsend_sem, xrecv_sems.at[i],
                                       device_id=xpeer, device_id_type=MESH) for i in range(NF)]

    for i in range(NF + NP):
        loads[i].wait()
        chunk(send, i)[...] = chunk(x_own, i)[...].astype(jnp.bfloat16)
        if i == 0:
            pl.semaphore_wait(barrier, jnp.where(is_b, 1, 2))
        ys[i].start()
        if i == 0:
            @pl.when(is_d)
            def _():
                pl.semaphore_signal(ready_sem, 1, device_id=xpeer, device_id_type=MESH)

    def add(local, remote, i, r):
        s = chunk(local, i)[...] + chunk(remote, i)[...].astype(jnp.float32)
        o_ref[pl.ds(r, ROWS), :] = s.astype(o_ref.dtype)

    for t in range(NF + max(NP, LAG)):
        if t < NF + NP:
            ys[t].wait_recv()
            if t == 0:
                @pl.when(is_b)
                def _():
                    pl.semaphore_wait(ready_sem, 1)
            if t < NF:
                xs[t].start()
            add(x_own, recv_y, t, row0(t))
        j = t - LAG
        if 0 <= j < NF:
            if j == 0:
                load_other.wait()
            xs[j].wait_recv()
            add(x_other, recv_x, j, pl.multiple_of(other0 + j * ROWS, ROWS))

    pltpu.make_async_copy(send, send, ysend_sem).wait()
    pltpu.make_async_copy(recv_x, recv_x, xsend_sem).wait()


def pallas_dist_ar_xy_y_m1024_n512_kernel(x: jax.Array):
    n_own, n_other = (NF + NP) * ROWS, NF * ROWS
    return pl.pallas_call(
        _body,
        out_shape=pltpu.VMEM((M, N), jnp.bfloat16),
        in_specs=[pl.BlockSpec(memory_space=pltpu.HBM)],
        out_specs=pl.BlockSpec(memory_space=pltpu.VMEM),
        scratch_shapes=[
            pltpu.VMEM((n_own, N), jnp.float32),
            pltpu.VMEM((n_other, N), jnp.float32),
            pltpu.VMEM((n_own, N), jnp.bfloat16),
            pltpu.VMEM((n_own, N), jnp.bfloat16),
            pltpu.VMEM((n_other, N), jnp.bfloat16),
            pltpu.SemaphoreType.DMA((NF + NP + 1,)),
            pltpu.SemaphoreType.DMA,
            pltpu.SemaphoreType.DMA((NF + NP,)),
            pltpu.SemaphoreType.DMA,
            pltpu.SemaphoreType.DMA((NF,)),
            pltpu.SemaphoreType.REGULAR,
        ],
        compiler_params=pltpu.CompilerParams(
            collective_id=0, disable_bounds_checks=True, disable_semaphore_checks=True),
    )(x)
```

```python
import jax
import jax.numpy as jnp
from jax import lax
from jax.experimental import pallas as pl
from jax.experimental.pallas import tpu as pltpu

M, N = 1024, 512
ROWS = 16
F_BLOCKS, P_BLOCKS = 28, 8
OWN_BLOCKS = F_BLOCKS + P_BLOCKS
F_UNITS = 2 * F_BLOCKS
P_UNITS = 2 * P_BLOCKS - 1
UNITS = F_UNITS + P_UNITS
SAMPLE = 4

STREAMS = ((F_BLOCKS, 5), (F_BLOCKS, 5), (P_UNITS, 2))
TAIL = 3
POOL_F, POOL_ALL = 19, 27
F_PLANES, F_POOL, F_WORDS = 10, 17, 19
P_PLANES, P_POOL, P_WORDS = 2, 4, 5

EARLY = 30
PREPARED = 58
START_A, START_C = 57, 33
RELAY_GROUPS = (32, 8, 6, 4, 2, 2, 1, 1)

I32 = jnp.int32
MESH = pl.DeviceIdType.MESH
ONES = 0x01010101


def _s32(v):
    return v - (1 << 32) if v >= (1 << 31) else v


TOP = _s32(0x80000000)
SIGN_MANTISSA = _s32(0x807F807F)


def _cdiv(a, b):
    return -(-a // b)


def _chunks(lo, hi, size):
    return [(k, min(size, hi - k)) for k in range(lo, hi, size)]


def _shl(a, b):
    return lax.shift_left(a, jnp.full(a.shape, b, I32) if isinstance(b, int) else b)


def _shr(a, b):
    return lax.shift_right_logical(a, jnp.full(a.shape, b, I32) if isinstance(b, int) else b)


def _sublane():
    return lax.broadcasted_iota(I32, (8, 128), 0)


def _at_least(v, k, bit):
    return _shr(v + _s32((0x80 - k) * ONES), 7 - bit) & (ONES << bit)


def _sum_above(v):
    acc = v
    for d in (1, 2, 4):
        acc = acc + jnp.where(_sublane() >= d, pltpu.roll(acc, d, 0), 0)
    return acc - v, jnp.broadcast_to(acc[7:8, :], v.shape)


def _centre(level):
    centre = _shr(level + 64, 7)
    return (centre + 2) * ONES, (128 * centre - level) * 0x00010001


def _split(lo, hi):
    rest = hi & SIGN_MANTISSA
    return ((lo & SIGN_MANTISSA) | _shl(rest, 8) | _shr(rest, 24),
            (_shr(lo, 7) & 0x00FF00FF) | (_shl(hi, 1) & _s32(0xFF00FF00)))


def _join(w, e):
    return ((w & SIGN_MANTISSA) | _shl(e & 0x00FF00FF, 7),
            ((_shr(w, 8) | _shl(w, 24)) & SIGN_MANTISSA) | _shr(e & _s32(0xFF00FF00), 1))


def _rank_plus_2(d):
    return (d + 10 * ONES - _at_least(d, 1, 2) - 3 * _at_least(d, 2, 1)
            + _at_least(d, 7, 0) + _at_least(d, 9, 0))


def _distance_minus_2(r):
    return (r - 3 * _at_least(r, 5, 1) + 5 * _at_least(r, 6, 0)
            - 9 * _at_least(r, 8, 0) + _at_least(r, 9, 3))


def _push(stream, ends, n_words, last):
    mark = jnp.full(ends.shape, TOP, I32)
    if last:
        ends = ends - ONES
    first = _shr(mark, ends & 31) | _shr(mark, _shr(ends, 8) & 31) | _shr(mark, _shr(ends, 16) & 31)
    if not last:
        first = first | mark
    down = _shr(ends, 24) & 31
    up = (32 - down) & 31
    out = [first | _shr(stream[0], down)]
    for k in range(1, n_words):
        v = _shl(stream[k - 1], up)
        out.append(v | _shr(stream[k], down) if k < len(stream) else v)
    return out


def _pop(stream, n_words, first):
    w, zeros = stream[0], []
    for k in range(4):
        if k or not first:
            w = _shl(w, 1)
        zeros.append(lax.clz(w))
        w = _shl(w, zeros[k])
    up = (zeros[0] + zeros[1]) + (zeros[2] + (3 if first else 4)) + zeros[3]
    down = 32 - up
    out = []
    for k in range(n_words):
        v = _shl(stream[k], up) if k else w
        out.append(v | _shr(stream[k + 1], down) if k + 1 < len(stream) else v)
    return zeros[0] | _shl(zeros[1], 8) | _shl(zeros[2], 16) | _shl(zeros[3], 24), out


def _words_needed(s, held):
    units, in_place = STREAMS[s]
    return min(_cdiv(1 + 31 * held, 32), _cdiv(32 * (in_place + TAIL) + 1 - 4 * (units - held), 32))


def _spread(tail, start, n_rows):
    row, bit = _shr(start, 5), start & 31
    moved = [(_shr(tail[k], bit) if k < TAIL else 0)
             | (_shl(_shl(tail[k - 1], 1), 31 - bit) if k else 0) for k in range(TAIL + 1)]
    out = []
    for k in range(n_rows):
        v = jnp.zeros_like(start)
        for d in range(min(TAIL, k) + 1):
            v = jnp.where(row == k - d, moved[d], v)
        out.append(v)
    return out


def _or_sublanes(v):
    for d in (4, 2, 1):
        v = [jnp.where((_sublane() & d) == 0, v[k] | pltpu.roll(v[k], 8 - d, 0),
                       v[k + d] | pltpu.roll(v[k + d], d, 0)) for k in range(d)]
    return v[0]


def _find_tail(rows, count):
    zero = jnp.zeros_like(count)
    rows = rows + [zero] * TAIL
    window, ones, before = rows[:TAIL + 1], zero, zero
    for k in range(len(rows) - TAIL - 1):
        ones = ones + lax.population_count(rows[k])
        passed = ones < count
        window = [jnp.where(passed, rows[k + 1 + d], window[d]) for d in range(TAIL + 1)]
        before = jnp.where(passed, ones, before)
    count = count - before
    low = zero + 32
    for step in (16, 8, 4, 2, 1):
        low = jnp.where(lax.population_count(_shr(window[0], low - step)) < count, low - step, low)
    return [_shl(_shl(window[d], 32 - low), 1) | _shr(window[d + 1], low - 1) for d in range(TAIL)]


def _words(ref, first, n=1):
    return ref.at[pl.ds(8 * first, 8 * n)]


def _slab(ref, unit, row=None):
    return ref.at[pl.ds(ROWS * (unit // 2) if row is None else row, ROWS), pl.ds(256 * (unit % 2), 256)]


def _either(coded, if_coded, if_raw):
    pl.when(coded)(if_coded)
    pl.when(jnp.logical_not(coded))(if_raw)


class _Messages:
    def __init__(self, byte, exp, hdr, exp_f, exp_p=None):
        self.byte, self.exp, self.hdr, self.exp_f, self.exp_p = byte, exp, hdr, exp_f, exp_p

    def in_place(self, s, k):
        return _words(self.exp_f, STREAMS[0][1] * s + k) if s < 2 else _words(self.exp_p, k)

    def plane(self, unit):
        if unit < F_UNITS:
            return _words(self.exp_f, F_PLANES + unit // 8), unit % 8
        return _words(self.exp_p, P_PLANES + (unit - F_UNITS) // 8), (unit - F_UNITS) % 8

    def pool_row(self, k):
        if k < 16:
            return self.exp_f.at[pl.ds(8 * F_POOL + k, 1)]
        if k < POOL_F:
            return self.hdr.at[pl.ds(k - 16, 1)]
        return self.exp_p.at[pl.ds(8 * P_POOL + k - POOL_F, 1)]

    def header(self):
        h = self.hdr[pl.ds(POOL_F - 16, 1), :]
        return (*_centre(jnp.broadcast_to(_shr(h, 1), (8, 128))), (h[0, 0] & 1) != 0)


class _Link:
    def __init__(self, src, dst, send_sems, recv_sems, peer, byte_groups):
        self.src, self.dst, self.peer, self.groups = src, dst, peer, byte_groups
        self.send_sems, self.recv_sems = send_sems, recv_sems

    def copy(self, src, dst, send, recv):
        return pltpu.make_async_remote_copy(
            src, dst, self.send_sems.at[send], self.recv_sems.at[recv],
            device_id=self.peer, device_id_type=MESH)

    def byte(self, first, n=1):
        group = max(g for g, (lo, _) in enumerate(self.groups) if lo <= first)
        return self.copy(_words(self.src.byte, first, n), _words(self.dst.byte, first, n),
                         0 if first < UNITS - 1 else 5, 3 + F_WORDS + group)

    def hdr(self):
        return self.copy(self.src.hdr, self.dst.hdr, 1, 0)

    def coded_f(self, k, n=1):
        return self.copy(_words(self.src.exp_f, k, n), _words(self.dst.exp_f, k, n), 2, 3 + k)

    def raw_f(self, k, n=1):
        lo, hi = F_UNITS * k // F_WORDS, F_UNITS * (k + n) // F_WORDS
        return self.copy(_words(self.src.exp, lo, hi - lo), _words(self.dst.exp, lo, hi - lo), 2, 3 + k)

    def coded_p(self):
        return self.copy(self.src.exp_p, self.dst.exp_p, 3, 1)

    def raw_p(self):
        return self.copy(_words(self.src.exp, F_UNITS, P_UNITS), _words(self.dst.exp, F_UNITS, P_UNITS), 3, 1)


class _Encoder:
    def __init__(self, out):
        zero = jnp.zeros((8, 128), I32)
        self.out = out
        self.streams = [[zero + TOP] for _ in STREAMS]
        self.held = [0] * len(STREAMS)
        self.length = [zero] * len(STREAMS)
        self.seen = self.magnitude = zero
        self.waiting, self.pool = [], []

    def split(self, unit, lo, hi):
        if unit < SAMPLE:
            both = (lo & 0x7FFF7FFF) + (hi & 0x7FFF7FFF)
            self.magnitude = self.magnitude + (both & 0xFFFF) + _shr(both, 16)
        else:
            lo, hi = lo + self.nudge, hi + self.nudge
        w, e = _split(lo, hi)
        _words(self.out.byte, unit)[...] = w
        _words(self.out.exp, unit)[...] = e
        self.waiting.append((unit, e))

    def code(self):
        unit = self.waiting[-1][0]
        if unit < SAMPLE - 1:
            return
        if unit == SAMPLE - 1:
            total = jnp.sum(jnp.sum(self.magnitude, axis=0, keepdims=True), axis=1, keepdims=True)
            self.level = _shr(jnp.broadcast_to(total, (8, 128)), (4096 * SAMPLE).bit_length() - 1) + 110
            self.offset, self.nudge = _centre(self.level)
        for unit, e in self.waiting:
            distance = self.offset - e
            rank = _rank_plus_2(distance)
            ends = (_shr(rank, 1) & (31 * ONES)) * ONES
            self.seen = self.seen | (distance | ends)
            plane, bit = self.out.plane(unit)
            self.plane = self.plane | _shl(rank & ONES, bit) if bit else rank & ONES
            if bit == 7 or unit == UNITS - 1:
                plane[...] = self.plane
            s = unit % 2 if unit < F_UNITS else 2
            self.held[s] += 1
            self.length[s] = self.length[s] + _shr(ends, 24)
            self.streams[s] = _push(self.streams[s], ends, _words_needed(s, self.held[s]),
                                    self.held[s] == STREAMS[s][0])
        self.waiting = []

    def check(self):
        misfit = self.seen & _s32(0xE0 * ONES)
        used, self.start = 1, []
        for s, (_, in_place) in enumerate(STREAMS):
            tail = jnp.maximum(self.length[s] - 32 * in_place, 0)
            above, total = _sum_above(tail)
            self.start.append(used + above)
            used = used + total
            room = (32 * TAIL - tail) | (32 * (POOL_F if s < 2 else POOL_ALL) - used)
            misfit = misfit | (room & TOP)
        misfit = jnp.max(jnp.where(misfit != 0, 1.0, 0.0), axis=0, keepdims=True)
        self.misfit = jnp.max(misfit, axis=1, keepdims=True)

    def close(self, s):
        if s == 0:
            self.coded = self.misfit[0, 0] == 0.0
        in_place = STREAMS[s][1]
        for k in range(in_place):
            self.out.in_place(s, k)[...] = self.streams[s][k]
        rows = _spread(self.streams[s][in_place:], self.start[s], POOL_F if s < 2 else POOL_ALL)
        self.pool = [v | self.pool[k] if k < len(self.pool) else v for k, v in enumerate(rows)]

    def seal(self):
        out, pool = self.out, self.pool
        _words(out.exp_f, F_POOL)[...] = _or_sublanes(pool[:8]) | jnp.where(_sublane() == 0, TOP, 0)
        _words(out.exp_f, F_POOL + 1)[...] = _or_sublanes(pool[8:16])
        out.hdr[pl.ds(0, POOL_F - 16), :] = _or_sublanes(pool[16:24])[:POOL_F - 16, :]
        _words(out.exp_p, P_POOL)[...] = _or_sublanes(pool[POOL_F:])
        out.hdr[pl.ds(POOL_F - 16, 1), :] = _shl(self.level[0:1, :], 1) | self.coded.astype(I32)


def _fetch_tail(msg, s, state):
    count = 1
    for k, (units, in_place) in enumerate(STREAMS[:s + 1]):
        ones = sum(lax.population_count(msg.in_place(k, j)[...]) for j in range(in_place))
        above, total = _sum_above(4 * units - ones)
        count = count + (above if k == s else total)
    rows = [jnp.broadcast_to(msg.pool_row(k)[...], (8, 128)) for k in range(POOL_F if s < 2 else POOL_ALL)]
    for k, v in enumerate(_find_tail(rows, count)):
        _words(state, 8 * s + k)[...] = v


def _decode(msg, offset, s, hi, lo, state):
    units, in_place = STREAMS[s]
    if hi == units:
        stream = [msg.in_place(s, k)[...] for k in range(in_place)]
        stream += [_words(state, 8 * s + k)[...] for k in range(TAIL)]
    else:
        stream = [_words(state, 8 * s + k)[...] for k in range(_words_needed(s, hi))]
    for i in reversed(range(lo, hi)):
        unit = 2 * i + s if s < 2 else F_UNITS + i
        zeros, stream = _pop(stream, min(_words_needed(s, i), in_place + TAIL), i == units - 1)
        plane, bit = msg.plane(unit)
        rank = _shl(zeros, 1) | ((_shr(plane[...], bit) if bit else plane[...]) & ONES)
        _words(msg.exp, unit)[...] = (offset - 2 * ONES) - _distance_minus_2(rank)
    if lo:
        for k, v in enumerate(stream):
            _words(state, 8 * s + k)[...] = v


Y_GROUPS = _chunks(0, F_UNITS, 1) + _chunks(F_UNITS, UNITS - 1, 2) + [(UNITS - 1, 1)]
X_GROUPS = [(sum(RELAY_GROUPS[:g]), n) for g, n in enumerate(RELAY_GROUPS)]
LOADS = [(0, 1), (1, 1)] + _chunks(2, 2 * OWN_BLOCKS, 2)


def _body(x_hbm, o_ref, own, other, mine, from_y, from_x, state, last_out, last_in, head_in,
          load_sems, y_send, y_recv, x_send, x_recv, ready):
    mine, from_y, from_x = _Messages(*mine), _Messages(*from_y), _Messages(*from_x)
    mx, my = lax.axis_index("x"), lax.axis_index("y")
    y_peer, x_peer = (mx, 1 - my), (1 - mx, my)
    is_a, is_b = (mx == 0) & (my == 0), (mx == 0) & (my == 1)
    is_c, is_d = (mx == 1) & (my == 0), (mx == 1) & (my == 1)
    y = _Link(mine, from_y, y_send, y_recv, y_peer, Y_GROUPS)
    x = _Link(from_y, from_x, x_send, x_recv, x_peer, X_GROUPS)

    def own_row(unit):
        row = ROWS * (unit // 2)
        return pl.multiple_of(mx * (ROWS * OWN_BLOCKS) + row, ROWS) if unit < F_UNITS else row

    def other_row(unit):
        return pl.multiple_of((1 - mx) * (ROWS * OWN_BLOCKS) + ROWS * (unit // 2), ROWS)

    def load(k):
        unit, n = LOADS[k]
        if n == 1:
            return pltpu.make_async_copy(_slab(x_hbm, unit, own_row(unit)), _slab(own, unit), load_sems.at[k])
        return pltpu.make_async_copy(x_hbm.at[pl.ds(own_row(unit), ROWS)],
                                     own.at[pl.ds(ROWS * (unit // 2), ROWS)], load_sems.at[k])

    def load_other():
        return pltpu.make_async_copy(x_hbm.at[pl.ds(other_row(0), ROWS * F_BLOCKS)], other,
                                     load_sems.at[len(LOADS)])

    def head():
        return y.copy(_slab(x_hbm, UNITS), head_in, 4, 2)

    def last():
        return y.copy(last_out, last_in, 4, 2)

    barrier = pltpu.get_barrier_semaphore()

    @pl.when(is_b)
    def _():
        pl.semaphore_wait(barrier, 1)
        head().start()

    load(0).start()
    pl.semaphore_signal(barrier, 1, device_id=y_peer, device_id_type=MESH)

    @pl.when(jnp.logical_not(is_d))
    def _():
        pl.semaphore_signal(barrier, 1, device_id=x_peer, device_id_type=MESH)

    for k in range(1, len(LOADS)):
        load(k).start()
    load_other().start()

    enc = _Encoder(mine)

    def send_bytes(groups):
        for first, n in groups:
            y.byte(first, n).start()

    def prepare(unit):
        for k, (first, _) in enumerate(LOADS):
            if first == unit:
                load(k).wait()
        rounded = _slab(own, unit)[...].astype(jnp.bfloat16)
        if unit == UNITS:
            last_out[...] = rounded
            return
        pairs = pltpu.bitcast(rounded, I32)
        enc.split(unit, pairs[:, :128], pairs[:, 128:])
        if unit == 0:
            pl.when(is_d)(lambda: pl.semaphore_wait(barrier, 2))
        if unit < EARLY and (unit < 4 or unit % 4 == 3 or unit == EARLY - 1):
            pl.when(my == 1)(lambda: send_bytes(Y_GROUPS[unit if unit < 4 else unit // 4 * 4:unit + 1]))
        if unit == 0:
            pl.when(is_d)(lambda: pl.semaphore_signal(ready, 1, device_id=x_peer, device_id_type=MESH))
        if unit in (START_A, START_C):
            @pl.when(is_a if unit == START_A else is_c)
            def _():
                pl.semaphore_wait(barrier, 2)
                send_bytes(Y_GROUPS[:EARLY])
        enc.code()

    def send_header():
        enc.seal()
        y.hdr().start()

    def send_exponents(first, n):
        def start(message):
            for k in range(first, first + n):
                message(k).start()
        _either(enc.coded, lambda: start(y.coded_f), lambda: start(y.raw_f))

    def send_middle():
        _either(enc.coded, lambda: y.coded_p().start(), lambda: y.raw_p().start())
        send_bytes(Y_GROUPS[F_UNITS:])
        pl.when(jnp.logical_not(is_b))(lambda: last().start())

    def relay(unit):
        y.byte(unit).wait_recv()
        if unit == 0:
            pl.when(is_b)(lambda: pl.semaphore_wait(ready, 1))
        x.byte(unit).start()

    for unit in range(PREPARED):
        prepare(unit)
    jobs = [lambda lo=lo, n=n: [prepare(u) for u in range(lo, lo + n)] for lo, n in _chunks(PREPARED, UNITS + 1, 3)]
    jobs += [enc.check] + [lambda s=s: enc.close(s) for s in range(3)] + [send_header]
    jobs += [lambda c=c: send_exponents(*c) for c in _chunks(0, F_WORDS, 5)]
    jobs += [lambda lo=lo, n=n: send_bytes(Y_GROUPS[lo:lo + n]) for lo, n in _chunks(EARLY, F_UNITS, 10)]
    jobs += [send_middle]
    for unit in range(EARLY):
        relay(unit)
        if jobs:
            jobs.pop(0)()
    assert not jobs

    def add(local, unit, row, remote):
        total = _slab(local, unit)[...] + remote.astype(jnp.float32)
        _slab(o_ref, unit, row)[...] = total.astype(o_ref.dtype)

    def merge(msg, nudge, local, unit, row):
        lo, hi = _join(_words(msg.byte, unit)[...], _words(msg.exp, unit)[...])
        if unit >= SAMPLE:
            lo, hi = lo - nudge, hi - nudge
        add(local, unit, row, pltpu.bitcast(jnp.concatenate([lo, hi], axis=1), jnp.bfloat16))

    def decode_f(msg, offset):
        steps = [lambda s=s: _fetch_tail(msg, s, state) for s in range(2)]
        for hi in range(F_BLOCKS, 0, -2):
            steps.append(lambda hi=hi: [_decode(msg, offset, s, hi, hi - 2, state) for s in range(2)] and None)
        return steps

    y.hdr().wait_recv()
    x.hdr().start()
    y_offset, y_nudge, y_coded = from_y.header()

    def relay_exponents(arriving, leaving):
        for k in range(F_WORDS):
            arriving(k).wait_recv()
            leaving(k).start()

    _either(y_coded, lambda: relay_exponents(y.coded_f, x.coded_f), lambda: relay_exponents(y.raw_f, x.raw_f))
    steps = decode_f(from_y, y_offset)
    pl.when(y_coded)(steps.pop(0))
    merged = 0
    for unit in range(EARLY, F_UNITS):
        relay(unit)
        if steps:
            pl.when(y_coded)(steps.pop(0))
        else:
            upto = min(merged + 6, unit + 1)
            for u in range(merged, upto):
                merge(from_y, y_nudge, own, u, own_row(u))
            merged = upto
    assert not steps and merged == F_UNITS

    def await_exponents(arriving):
        for k in range(F_WORDS):
            arriving(k).wait_recv()

    x.hdr().wait_recv()
    x_offset, x_nudge, x_coded = from_x.header()

    def decode_x():
        await_exponents(x.coded_f)
        for s in range(2):
            _fetch_tail(from_x, s, state)
        for step in decode_f(from_x, x_offset)[2:]:
            step()

    def decode_p():
        y.coded_p().wait_recv()
        _fetch_tail(from_y, 2, state)
        _decode(from_y, y_offset, 2, P_UNITS, 0, state)

    _either(x_coded, decode_x, lambda: await_exponents(x.raw_f))
    _either(y_coded, decode_p, lambda: y.raw_p().wait_recv())

    y.hdr().wait_send()
    x.hdr().wait_send()
    _either(enc.coded,
            lambda: (y.coded_f(0, F_WORDS).wait_send(), y.coded_p().wait_send()) and None,
            lambda: (y.raw_f(0, F_WORDS).wait_send(), y.raw_p().wait_send()) and None)
    _either(y_coded, lambda: x.coded_f(0, F_WORDS).wait_send(), lambda: x.raw_f(0, F_WORDS).wait_send())
    pl.when(is_b)(lambda: head().wait_send())
    load_other().wait()

    @pl.when(is_a)
    def _():
        head().wait_recv()
        add(own, UNITS, own_row(UNITS), head_in[...])

    left = [(F_UNITS - lo - n, 0, lo, n) for lo, n in X_GROUPS]
    left += [(UNITS - lo - n, 1, lo, n) for lo, n in Y_GROUPS[F_UNITS:]]
    left.sort(reverse=True)
    for k, (_, on_y, lo, n) in enumerate(left):
        if k == len(left) - 2:
            x.byte(0, F_UNITS).wait_send()
            y.byte(0, UNITS - 1).wait_send()
            y.byte(UNITS - 1).wait_send()
            pl.when(jnp.logical_not(is_b))(lambda: last().wait_send())
        (y if on_y else x).byte(lo, n).wait_recv()
        for u in range(lo, lo + n):
            if on_y:
                merge(from_y, y_nudge, own, u, own_row(u))
            else:
                merge(from_x, x_nudge, other, u, other_row(u))

    @pl.when(jnp.logical_not(is_a))
    def _():
        last().wait_recv()
        add(own, UNITS, own_row(UNITS), last_in[...])


def pallas_dist_ar_xy_y_m1024_n512_kernel(x: jax.Array):
    def words(n):
        return pltpu.VMEM((8 * n, 128), I32)

    def messages(units):
        f = [words(units), words(units), pltpu.VMEM((POOL_F - 15, 128), I32), words(F_WORDS)]
        return f + [words(P_WORDS)] if units > F_UNITS else f

    return pl.pallas_call(
        _body,
        out_shape=pltpu.VMEM((M, N), jnp.bfloat16),
        in_specs=[pl.BlockSpec(memory_space=pltpu.HBM)],
        out_specs=pl.BlockSpec(memory_space=pltpu.VMEM),
        scratch_shapes=[
            pltpu.VMEM((ROWS * OWN_BLOCKS, N), jnp.float32),
            pltpu.VMEM((ROWS * F_BLOCKS, N), jnp.float32),
            messages(UNITS),
            messages(UNITS),
            messages(F_UNITS),
            words(8 * len(STREAMS)),
            pltpu.VMEM((ROWS, 256), jnp.bfloat16),
            pltpu.VMEM((ROWS, 256), jnp.bfloat16),
            pltpu.VMEM((ROWS, 256), jnp.float32),
            pltpu.SemaphoreType.DMA((len(LOADS) + 1,)),
            pltpu.SemaphoreType.DMA((6,)),
            pltpu.SemaphoreType.DMA((3 + F_WORDS + len(Y_GROUPS),)),
            pltpu.SemaphoreType.DMA((3,)),
            pltpu.SemaphoreType.DMA((3 + F_WORDS + len(X_GROUPS),)),
            pltpu.SemaphoreType.REGULAR,
        ],
        compiler_params=pltpu.CompilerParams(
            collective_id=0, disable_bounds_checks=True, disable_semaphore_checks=True),
    )(x)
```

```python
import jax
import jax.numpy as jnp
import numpy as np
from jax import lax
from jax.experimental import pallas as pl
from jax.experimental.pallas import tpu as pltpu

M, N = 1024, 512
ROWS = 16
F_BLOCKS, P_BLOCKS = 28, 8
OWN_BLOCKS = F_BLOCKS + P_BLOCKS
F_UNITS = 2 * F_BLOCKS
P_UNITS = 2 * P_BLOCKS - 1
UNITS = F_UNITS + P_UNITS
SAMPLE = 4

F, P = 0, 1
WIDTH, PUSHES, IN_PLACE, POOL = (2, 1), (F_BLOCKS, P_UNITS), (5, 2), (19, 27)
TAIL = 3
F_PLANES, F_POOL, F_WORDS = 10, 17, 19
P_PLANES, P_POOL, P_WORDS = 2, 4, 5
HEADER_ROW = 3

EARLY = 32
PREPARED = 58
START_A, START_C = 56, 32
MERGED = 36
RELAY_GROUPS = (32, 8, 6, 4, 2, 2, 1, 1)

I32 = jnp.int32
MESH = pl.DeviceIdType.MESH
ONES = 0x01010101


def _s32(v):
    return v - (1 << 32) if v >= (1 << 31) else v


TOP = _s32(0x80000000)
SIGN_MANTISSA = _s32(0x807F807F)


def _cdiv(a, b):
    return -(-a // b)


def _chunks(lo, hi, size):
    return [(k, min(size, hi - k)) for k in range(lo, hi, size)]


def _shl(a, b):
    return lax.shift_left(a, np.int32(b) if isinstance(b, int) else b)


def _shr(a, b):
    return lax.shift_right_logical(a, np.int32(b) if isinstance(b, int) else b)


def _sublane(like):
    return lax.broadcasted_iota(I32, like.shape, 0)


def _at_least(v, k, bit):
    return _shr(v + _s32((0x80 - k) * ONES), 7 - bit) & (ONES << bit)


def _sum_above(v):
    acc, d = v, 1
    while d < v.shape[0]:
        acc = acc + jnp.where(_sublane(v) >= d, pltpu.roll(acc, d, 0), 0)
        d *= 2
    return acc - v, jnp.broadcast_to(acc[-1:, :], (8, 128))


def _centre(level):
    centre = _shr(level + 64, 7)
    return (centre + 2) * ONES, (128 * centre - level) * 0x00010001


def _split(lo, hi):
    rest = hi & SIGN_MANTISSA
    return ((lo & SIGN_MANTISSA) | _shl(rest, 8) | _shr(rest, 24),
            (_shr(lo, 7) & 0x00FF00FF) | (_shl(hi, 1) & _s32(0xFF00FF00)))


def _join(w, e):
    return ((w & SIGN_MANTISSA) | _shl(e & 0x00FF00FF, 7),
            ((_shr(w, 8) | _shl(w, 24)) & SIGN_MANTISSA) | _shr(e & _s32(0xFF00FF00), 1))


def _rank_plus_2(d):
    return (d + 10 * ONES - _at_least(d, 1, 2) - 3 * _at_least(d, 2, 1)
            + _at_least(d, 7, 0) + _at_least(d, 9, 0))


def _distance_minus_2(r):
    return (r - 3 * _at_least(r, 5, 1) + 5 * _at_least(r, 6, 0)
            - 9 * _at_least(r, 8, 0) + _at_least(r, 9, 3))


def _push(stream, ends, n_words, last):
    mark = jnp.full(ends.shape, TOP, I32)
    if last:
        ends = ends - ONES
    first = _shr(mark, ends & 31) | _shr(mark, _shr(ends, 8) & 31) | _shr(mark, _shr(ends, 16) & 31)
    if not last:
        first = first | mark
    down = _shr(ends, 24) & 31
    up = (32 - down) & 31
    out = [first | _shr(stream[0], down)]
    for k in range(1, n_words):
        v = _shl(stream[k - 1], up)
        out.append(v | _shr(stream[k], down) if k < len(stream) else v)
    return out


def _pop(stream, n_words, first):
    w, zeros = stream[0], []
    for k in range(4):
        if k or not first:
            w = _shl(w, 1)
        zeros.append(lax.clz(w))
        w = _shl(w, zeros[k])
    up = (zeros[0] + zeros[1]) + (zeros[2] + (3 if first else 4)) + zeros[3]
    down = 32 - up
    out = []
    for k in range(n_words):
        v = _shl(stream[k], up) if k else w
        out.append(v | _shr(stream[k + 1], down) if k + 1 < len(stream) else v)
    return zeros[0] | _shl(zeros[1], 8) | _shl(zeros[2], 16) | _shl(zeros[3], 24), out


def _words_needed(part, held):
    room = 32 * (IN_PLACE[part] + TAIL) + 1 - 4 * (PUSHES[part] - held)
    return _cdiv(min(1 + 31 * held, room), 32)


def _spread(tail, start, n_rows):
    row, bit = _shr(start, 5), start & 31
    moved = [(_shr(tail[k], bit) if k < TAIL else 0)
             | (_shl(_shl(tail[k - 1], 1), 31 - bit) if k else 0) for k in range(TAIL + 1)]
    here = [row == k for k in range(n_rows)]
    out = []
    for k in range(n_rows):
        v = jnp.zeros_like(start)
        for d in range(min(TAIL, k) + 1):
            v = lax.select(here[k - d], moved[d], v)
        out.append(v)
    return out


def _or_sublanes(v):
    for d in (4, 2, 1):
        v = [jnp.where((_sublane(v[0]) & d) == 0, v[k] | pltpu.roll(v[k], 8 - d, 0),
                       v[k + d] | pltpu.roll(v[k + d], d, 0)) for k in range(d)]
    return v[0]


def _find_tail(rows, count):
    zero = jnp.zeros_like(count)
    rows = rows + [zero] * TAIL
    window, ones, before = rows[:TAIL + 1], zero, zero
    for k in range(len(rows) - TAIL - 1):
        ones = ones + lax.population_count(rows[k])
        passed = ones < count
        window = [lax.select(passed, rows[k + 1 + d], window[d]) for d in range(TAIL + 1)]
        before = lax.select(passed, ones, before)
    count = count - before
    low = zero + 32
    for step in (16, 8, 4, 2, 1):
        low = lax.select(lax.population_count(_shr(window[0], low - step)) < count, low - step, low)
    return [_shl(_shl(window[d], 32 - low), 1) | _shr(window[d + 1], low - 1) for d in range(TAIL)]


def _words(ref, first, n=1):
    return ref.at[pl.ds(8 * first, 8 * n)]


def _slab(ref, unit, n=1, row=None):
    return ref.at[pl.ds(ROWS * (unit // 2) if row is None else row, ROWS), pl.ds(256 * (unit % 2), 256 * n)]


def _either(coded, if_coded, if_raw):
    pl.when(coded)(if_coded)
    pl.when(jnp.logical_not(coded))(if_raw)


class _Messages:
    def __init__(self, byte, exp, hdr, exp_f, exp_p=None):
        self.byte, self.exp, self.hdr, self.exp_f, self.exp_p = byte, exp, hdr, exp_f, exp_p

    def in_place(self, part, k):
        return _words(self.exp_p, k) if part == P else _words(self.exp_f, 2 * k, 2)

    def plane(self, unit):
        if unit < F_UNITS:
            return _words(self.exp_f, F_PLANES + unit // 8), unit % 8
        return _words(self.exp_p, P_PLANES + (unit - F_UNITS) // 8), (unit - F_UNITS) % 8

    def pool_row(self, k):
        if k < 16:
            return self.exp_f.at[pl.ds(8 * F_POOL + k, 1)]
        if k < POOL[F]:
            return self.hdr.at[pl.ds(k - 16, 1)]
        return self.exp_p.at[pl.ds(8 * P_POOL + k - POOL[F], 1)]

    def header(self):
        h = self.hdr[pl.ds(HEADER_ROW, 1), :]
        return (*_centre(_shr(h, 1)), (h[0, 0] & 1) != 0)


class _Link:
    def __init__(self, src, dst, send_sems, recv_sems, peer, byte_groups, exp_sems):
        self.src, self.dst, self.peer = src, dst, peer
        self.groups, self.exp_sems = byte_groups, exp_sems
        self.send_sems, self.recv_sems = send_sems, recv_sems

    def copy(self, src, dst, send, recv):
        return pltpu.make_async_remote_copy(
            src, dst, self.send_sems.at[send], self.recv_sems.at[recv],
            device_id=self.peer, device_id_type=MESH)

    def byte(self, first, n=1):
        group = max(g for g, (lo, _) in enumerate(self.groups) if lo <= first)
        return self.copy(_words(self.src.byte, first, n), _words(self.dst.byte, first, n),
                         0 if first < UNITS - 1 else 5, 3 + self.exp_sems + group)

    def hdr(self):
        return self.copy(self.src.hdr, self.dst.hdr, 1, 0)

    def coded_f(self, k, n=1):
        return self.copy(_words(self.src.exp_f, k, n), _words(self.dst.exp_f, k, n),
                         2, 3 + k % self.exp_sems)

    def raw_f(self, k, n=1):
        lo, hi = F_UNITS * k // F_WORDS, F_UNITS * (k + n) // F_WORDS
        return self.copy(_words(self.src.exp, lo, hi - lo), _words(self.dst.exp, lo, hi - lo),
                         2, 3 + k % self.exp_sems)

    def coded_p(self):
        return self.copy(self.src.exp_p, self.dst.exp_p, 3, 1)

    def raw_p(self):
        return self.copy(_words(self.src.exp, F_UNITS, P_UNITS), _words(self.dst.exp, F_UNITS, P_UNITS), 3, 1)


class _Encoder:
    def __init__(self, out):
        self.out = out
        self.length = [jnp.zeros((8 * width, 128), I32) for width in WIDTH]
        self.streams = [[zero + TOP] for zero in self.length]
        self.seen = list(self.length)
        self.held = [0, 0]
        self.magnitude = 0
        self.waiting, self.start, self.pool = [], [], []

    def split(self, unit, n, pairs):
        lo, hi = [jnp.concatenate([pairs[:, c:c + 128] for c in range(half, 256 * n, 256)])
                  for half in (0, 128)]
        if unit >= SAMPLE:
            lo, hi = lo + self.nudge, hi + self.nudge
        w, e = _split(lo, hi)
        _words(self.out.byte, unit, n)[...] = w
        _words(self.out.exp, unit, n)[...] = e
        self.waiting += [e[8 * k:8 * k + 8] for k in range(n)]
        if unit < SAMPLE:
            both = (lo & 0x7FFF7FFF) + (hi & 0x7FFF7FFF)
            both = (both & 0xFFFF) + _shr(both, 16)
            self.magnitude = self.magnitude + sum(both[8 * k:8 * k + 8] for k in range(n))

    def code(self, split_units):
        if split_units < SAMPLE:
            return
        if split_units == SAMPLE:
            total = jnp.sum(jnp.sum(self.magnitude, axis=0, keepdims=True), axis=1, keepdims=True)
            self.level = _shr(jnp.broadcast_to(total, (1, 128)), (4096 * SAMPLE).bit_length() - 1) + 110
            self.offset, self.nudge = _centre(self.level)
        while self.waiting:
            unit = split_units - len(self.waiting)
            part = F if unit < F_UNITS else P
            n = WIDTH[part]
            distance = self.offset - jnp.concatenate(self.waiting[:n])
            del self.waiting[:n]
            rank = _rank_plus_2(distance)
            ends = (_shr(rank, 1) & (63 * ONES)) * ONES
            self.seen[part] = self.seen[part] | ((distance & _s32(0xC0 * ONES)) | ends)
            low = rank & ONES
            for k in range(n):
                plane, bit = self.out.plane(unit + k)
                self.plane = self.plane | _shl(low[8 * k:8 * k + 8], bit) if bit else low[:8]
                if bit == 7 or unit + k == UNITS - 1:
                    plane[...] = self.plane
            self.held[part] += 1
            self.length[part] = self.length[part] + _shr(ends, 24)
            self.streams[part] = _push(self.streams[part], ends, _words_needed(part, self.held[part]),
                                       self.held[part] == PUSHES[part])

    def check(self):
        used, misfit = 1, []
        for part in (F, P):
            tail = jnp.maximum(self.length[part] - 32 * IN_PLACE[part], 0)
            above, total = _sum_above(tail)
            self.start.append(used + above)
            used = used + total
            misfit += [self.seen[part] & _s32(0xE0 * ONES),
                       (32 * TAIL - tail) & TOP, (32 * POOL[part] - used) & TOP]
        self.misfit = jnp.max(jnp.where(jnp.concatenate(misfit) != 0, 1.0, 0.0), axis=0, keepdims=True)

    def decide(self):
        self.misfit = jnp.max(self.misfit, axis=1, keepdims=True)

    def close(self, part, k):
        stream, rows = self.streams[part], slice(8 * k, 8 * k + 8)
        if k == 0:
            for j in range(IN_PLACE[part]):
                self.out.in_place(part, j)[...] = stream[j]
        if not self.pool:
            self.coded = self.misfit[0, 0] == 0.0
        added = _spread([v[rows] for v in stream[IN_PLACE[part]:]], self.start[part][rows], POOL[part])
        self.pool = [v | self.pool[j] if j < len(self.pool) else v for j, v in enumerate(added)]

    def seal(self):
        out, pool = self.out, self.pool
        _words(out.exp_f, F_POOL)[...] = _or_sublanes(pool[:8]) | jnp.where(_sublane(pool[0]) == 0, TOP, 0)
        _words(out.exp_f, F_POOL + 1)[...] = _or_sublanes(pool[8:16])
        out.hdr[pl.ds(0, HEADER_ROW), :] = _or_sublanes(pool[16:24])[:HEADER_ROW, :]
        _words(out.exp_p, P_POOL)[...] = _or_sublanes(pool[POOL[F]:])
        out.hdr[pl.ds(HEADER_ROW, 1), :] = _shl(self.level, 1) | self.coded.astype(I32)


def _fetch_tail(msg, part, k, state):
    count = 1
    for earlier in range(part + 1):
        ones = sum(lax.population_count(msg.in_place(earlier, j)[...]) for j in range(IN_PLACE[earlier]))
        above, total = _sum_above(4 * PUSHES[earlier] - ones)
        count = count + (above[8 * k:8 * k + 8] if earlier == part else total)
    rows = [jnp.broadcast_to(msg.pool_row(j)[...], (8, 128)) for j in range(POOL[part])]
    for j, v in enumerate(_find_tail(rows, count)):
        _words(state, 2 * j + k)[...] = v


def _decode(msg, offset, part, hi, lo, state):
    n = WIDTH[part]
    if hi == PUSHES[part]:
        stream = [msg.in_place(part, j)[...] for j in range(IN_PLACE[part])]
        stream += [_words(state, 2 * j, n)[...] for j in range(TAIL)]
    else:
        stream = [_words(state, 2 * j, n)[...] for j in range(_words_needed(part, hi))]
    for i in reversed(range(lo, hi)):
        unit = 2 * i if part == F else F_UNITS + i
        zeros, stream = _pop(stream, min(_words_needed(part, i), len(stream)), i == PUSHES[part] - 1)
        low = jnp.concatenate([_shr(plane[...], bit) for plane, bit in map(msg.plane, range(unit, unit + n))])
        rank = _shl(zeros, 1) | (low & ONES)
        _words(msg.exp, unit, n)[...] = (offset - 2 * ONES) - _distance_minus_2(rank)
    if lo:
        for j, v in enumerate(stream):
            _words(state, 2 * j, n)[...] = v


LOADS = [(0, 1), (1, 1)] + _chunks(2, 2 * OWN_BLOCKS, 2)
Y_GROUPS = _chunks(0, F_UNITS, 1) + _chunks(F_UNITS, UNITS, 2)
X_GROUPS = [(sum(RELAY_GROUPS[:g]), n) for g, n in enumerate(RELAY_GROUPS)]


def _body(x_hbm, o_ref, own, other, mine, from_y, from_x, state, last_out, last_in, head_in,
          load_sems, y_send, y_recv, x_send, x_recv, ready):
    mine, from_y, from_x = _Messages(*mine), _Messages(*from_y), _Messages(*from_x)
    mx, my = lax.axis_index("x"), lax.axis_index("y")
    y_peer, x_peer = (mx, 1 - my), (1 - mx, my)
    is_a, is_b = (mx == 0) & (my == 0), (mx == 0) & (my == 1)
    is_c, is_d = (mx == 1) & (my == 0), (mx == 1) & (my == 1)
    y = _Link(mine, from_y, y_send, y_recv, y_peer, Y_GROUPS, F_WORDS)
    x = _Link(from_y, from_x, x_send, x_recv, x_peer, X_GROUPS, 1)

    def own_row(unit):
        row = ROWS * (unit // 2)
        return pl.multiple_of(mx * (ROWS * OWN_BLOCKS) + row, ROWS) if unit < F_UNITS else row

    def other_row(unit):
        return pl.multiple_of((1 - mx) * (ROWS * OWN_BLOCKS) + ROWS * (unit // 2), ROWS)

    def load(k):
        unit, n = LOADS[k]
        return pltpu.make_async_copy(_slab(x_hbm, unit, n, own_row(unit)), _slab(own, unit, n), load_sems.at[k])

    def load_other():
        return pltpu.make_async_copy(x_hbm.at[pl.ds(other_row(0), ROWS * F_BLOCKS)], other,
                                     load_sems.at[len(LOADS)])

    def head():
        return y.copy(_slab(x_hbm, UNITS), head_in, 4, 2)

    def last():
        return y.copy(last_out, last_in, 4, 2)

    barrier = pltpu.get_barrier_semaphore()

    @pl.when(is_b)
    def _():
        pl.semaphore_wait(barrier, 1)
        head().start()

    load(0).start()
    pl.semaphore_signal(barrier, 1, device_id=y_peer, device_id_type=MESH)

    @pl.when(jnp.logical_not(is_d))
    def _():
        pl.semaphore_signal(barrier, 1, device_id=x_peer, device_id_type=MESH)

    for k in range(1, len(LOADS)):
        load(k).start()
    load_other().start()

    enc = _Encoder(mine)

    def send_bytes(groups):
        for first, n in groups:
            y.byte(first, n).start()

    def prepare(k):
        unit, n = LOADS[k]
        load(k).wait()
        rounded = _slab(own, unit, n)[...].astype(jnp.bfloat16)
        if unit + n > UNITS:
            last_out[...] = rounded[:, 256:]
            n = 1
        enc.split(unit, n, pltpu.bitcast(rounded, I32))
        if unit == 0:
            pl.when(is_d)(lambda: pl.semaphore_wait(barrier, 2))
        if unit < EARLY:
            pl.when(my == 1)(lambda: send_bytes(Y_GROUPS[unit:unit + n]))
        if unit == 0:
            pl.when(is_d)(lambda: pl.semaphore_signal(ready, 1, device_id=x_peer, device_id_type=MESH))
        if unit in (START_A, START_C):
            @pl.when(is_a if unit == START_A else is_c)
            def _():
                pl.semaphore_wait(barrier, 2)
                send_bytes(Y_GROUPS[:EARLY])
        enc.code(unit + n)

    def send_header():
        enc.seal()
        y.hdr().start()

    def send_exponents(first, n):
        def start(message):
            for k in range(first, first + n):
                message(k).start()
        _either(enc.coded, lambda: start(y.coded_f), lambda: start(y.raw_f))

    def send_middle():
        _either(enc.coded, lambda: y.coded_p().start(), lambda: y.raw_p().start())
        send_bytes(Y_GROUPS[F_UNITS:])
        pl.when(jnp.logical_not(is_b))(lambda: last().start())

    def relay(unit):
        y.byte(unit).wait_recv()
        if unit == 0:
            pl.when(is_b)(lambda: pl.semaphore_wait(ready, 1))
        x.byte(unit).start()

    jobs = []
    for k, (unit, _) in enumerate(LOADS):
        if unit < PREPARED:
            prepare(k)
        else:
            jobs.append(lambda k=k: prepare(k))
    jobs += [enc.check, enc.decide, lambda: enc.close(F, 0), lambda: enc.close(F, 1),
             lambda: enc.close(P, 0), send_header]
    jobs += [lambda c=c: send_exponents(*c) for c in _chunks(0, F_WORDS, 5)]
    jobs += [lambda lo=lo, n=n: send_bytes(Y_GROUPS[lo:lo + n]) for lo, n in _chunks(EARLY, F_UNITS, 10)]
    jobs += [send_middle]
    assert START_C < START_A < PREPARED and len(jobs) <= EARLY <= START_C
    for unit in range(EARLY):
        relay(unit)
        if jobs:
            jobs.pop(0)()

    def add(local, unit, n, row, remote):
        total = _slab(local, unit, n)[...] + remote.astype(jnp.float32)
        _slab(o_ref, unit, n, row)[...] = total.astype(o_ref.dtype)

    def merge(msg, nudge, local, row_of, first, count):
        for unit, n in _chunks(first, first + count, 2):
            lo, hi = _join(_words(msg.byte, unit, n)[...], _words(msg.exp, unit, n)[...])
            if unit >= SAMPLE:
                lo, hi = lo - nudge, hi - nudge
            pairs = jnp.concatenate([v[8 * k:8 * k + 8] for k in range(n) for v in (lo, hi)], axis=1)
            add(local, unit, n, row_of(unit), pltpu.bitcast(pairs, jnp.bfloat16))

    def decode_f(msg, header):
        steps = [lambda k=k: _fetch_tail(msg, F, k, state) for k in range(2)]
        steps += [lambda hi=hi: _decode(msg, header[0], F, hi, hi - 2, state) for hi in range(F_BLOCKS, 0, -2)]
        return [lambda step=step: pl.when(header[2])(step) for step in steps]

    def relay_exponents(arriving, leaving):
        for k in range(F_WORDS):
            arriving(k).wait_recv()
            leaving(k).start()

    y.hdr().wait_recv()
    x.hdr().start()
    y_header = y_offset, y_nudge, y_coded = from_y.header()
    _either(y_coded, lambda: relay_exponents(y.coded_f, x.coded_f), lambda: relay_exponents(y.raw_f, x.raw_f))

    x_header = []

    def open_x():
        x.hdr().wait_recv()
        x_header.extend(from_x.header())

    def await_x():
        _either(x_header[2], lambda: x.coded_f(0, F_WORDS).wait_recv(), lambda: x.raw_f(0, F_WORDS).wait_recv())

    jobs = decode_f(from_y, y_header)
    jobs += [lambda c=c: merge(from_y, y_nudge, own, own_row, *c) for c in _chunks(0, MERGED, 10)]
    assert MERGED <= EARLY + len(jobs) - _cdiv(MERGED, 10)
    jobs += [open_x, await_x] + decode_f(from_x, x_header)
    for unit in range(EARLY, F_UNITS):
        jobs.pop(0)()
        relay(unit)
    for job in jobs:
        job()
    merge(from_y, y_nudge, own, own_row, MERGED, F_UNITS - MERGED)

    def decode_p():
        y.coded_p().wait_recv()
        _fetch_tail(from_y, P, 0, state)
        _decode(from_y, y_offset, P, P_UNITS, 0, state)

    _either(y_coded, decode_p, lambda: y.raw_p().wait_recv())

    y.hdr().wait_send()
    x.hdr().wait_send()
    _either(enc.coded, lambda: y.coded_f(0, F_WORDS).wait_send(), lambda: y.raw_f(0, F_WORDS).wait_send())
    _either(enc.coded, lambda: y.coded_p().wait_send(), lambda: y.raw_p().wait_send())
    _either(y_coded, lambda: x.coded_f(0, F_WORDS).wait_send(), lambda: x.raw_f(0, F_WORDS).wait_send())
    pl.when(is_b)(lambda: head().wait_send())
    load_other().wait()

    @pl.when(is_a)
    def _():
        head().wait_recv()
        add(own, UNITS, 1, own_row(UNITS), head_in[...])

    left = [(lo + n - F_UNITS, 0, lo, n) for lo, n in X_GROUPS]
    left += [(lo + n - UNITS, 1, lo, n) for lo, n in Y_GROUPS[F_UNITS:]]
    for k, (_, on_y, lo, n) in enumerate(sorted(left)):
        if k == len(left) - 2:
            x.byte(0, F_UNITS).wait_send()
            y.byte(0, UNITS - 1).wait_send()
            y.byte(UNITS - 1).wait_send()
            pl.when(jnp.logical_not(is_b))(lambda: last().wait_send())
        (y if on_y else x).byte(lo, n).wait_recv()
        if on_y:
            merge(from_y, y_nudge, own, own_row, lo, n)
        else:
            merge(from_x, x_header[1], other, other_row, lo, n)

    @pl.when(jnp.logical_not(is_a))
    def _():
        last().wait_recv()
        add(own, UNITS, 1, own_row(UNITS), last_in[...])


def pallas_dist_ar_xy_y_m1024_n512_kernel(x: jax.Array):
    def words(n):
        return pltpu.VMEM((8 * n, 128), I32)

    def messages(units):
        f = [words(units), words(units), pltpu.VMEM((HEADER_ROW + 1, 128), I32), words(F_WORDS)]
        return f + [words(P_WORDS)] if units > F_UNITS else f

    return pl.pallas_call(
        _body,
        out_shape=pltpu.VMEM((M, N), jnp.bfloat16),
        in_specs=[pl.BlockSpec(memory_space=pltpu.HBM)],
        out_specs=pl.BlockSpec(memory_space=pltpu.VMEM),
        scratch_shapes=[
            pltpu.VMEM((ROWS * OWN_BLOCKS, N), jnp.float32),
            pltpu.VMEM((ROWS * F_BLOCKS, N), jnp.float32),
            messages(UNITS),
            messages(UNITS),
            messages(F_UNITS),
            words(2 * (IN_PLACE[F] + TAIL)),
            pltpu.VMEM((ROWS, 256), jnp.bfloat16),
            pltpu.VMEM((ROWS, 256), jnp.bfloat16),
            pltpu.VMEM((ROWS, 256), jnp.float32),
            pltpu.SemaphoreType.DMA((len(LOADS) + 1,)),
            pltpu.SemaphoreType.DMA((6,)),
            pltpu.SemaphoreType.DMA((3 + F_WORDS + len(Y_GROUPS),)),
            pltpu.SemaphoreType.DMA((3,)),
            pltpu.SemaphoreType.DMA((4 + len(X_GROUPS),)),
            pltpu.SemaphoreType.REGULAR,
        ],
        compiler_params=pltpu.CompilerParams(
            collective_id=0, disable_semaphore_checks=True),
    )(x)
```
